```python
import numpy as np

kernel_name = "dist_layernorm_xy_m6144_n2048"

def setup_inputs():
    x = np.random.randn(12288, 4096).astype(np.float32)
    gamma = np.random.randn(4096).astype(np.float32)
    beta = np.random.randn(4096).astype(np.float32)
    return {"x": x, "gamma": gamma, "beta": beta}

def reference(x: np.ndarray, gamma: np.ndarray, beta: np.ndarray) -> np.ndarray:
    eps = 1e-5
    mean = np.mean(x, axis=1, keepdims=True)
    var = np.var(x, axis=1, keepdims=True)
    return gamma * (x - mean) / np.sqrt(var + eps) + beta
```

```python
import jax
import jax.numpy as jnp
from jax import lax
from jax.experimental import pallas as pl
from jax.experimental.pallas import tpu as pltpu

EPS = 1e-5
R = 256
D = 4
LAG = 1
CH = 64
NCH = 32


def pallas_dist_layernorm_xy_m6144_n2048_kernel(
    x: jax.Array,
    gamma: jax.Array,
    beta: jax.Array,
):
    M, N = x.shape
    NB = M // R
    n_total = 2 * N
    out_dtype = jnp.float32

    def body(x_hbm, g_hbm, b_hbm, o_ref,
             xbuf, gb1, gb, col, mu, rs, st_send, st_recv,
             rsem, gsem, ssem, vsem):
        my_x = lax.axis_index("x")
        my_y = lax.axis_index("y")
        peer = (my_x, 1 - my_y)

        def rd(i):
            return pltpu.make_async_copy(x_hbm.at[pl.ds(i * R, R), :], xbuf.at[i], rsem.at[i])

        def xch(i):
            return pltpu.make_async_remote_copy(
                src_ref=st_send.at[i], dst_ref=st_recv.at[i],
                send_sem=ssem.at[i], recv_sem=vsem.at[i],
                device_id=peer, device_id_type=pl.DeviceIdType.MESH)

        for i in range(min(D, NB)):
            rd(i).start()
        cg = pltpu.make_async_copy(g_hbm, gb1.at[0], gsem.at[0])
        cb = pltpu.make_async_copy(b_hbm, gb1.at[1], gsem.at[1])
        cg.start()
        cb.start()
        bar = pltpu.get_barrier_semaphore()
        pl.semaphore_signal(bar, inc=1, device_id=peer, device_id_type=pl.DeviceIdType.MESH)

        lane = lax.broadcasted_iota(jnp.int32, (CH, 128), 1)

        def stats(i):
            def chunk(c, _):
                r0 = pl.multiple_of(c * CH, CH)
                xs = xbuf[i, pl.ds(r0, CH), :]
                mean = jnp.sum(xs, axis=-1, keepdims=True) * (1.0 / N)
                d = xs - mean
                m2 = jnp.sum(d * d, axis=-1, keepdims=True)
                col[pl.ds(r0, CH), :] = jnp.where(lane < 64, mean, m2)
                return 0
            lax.fori_loop(0, R // CH, chunk, 0)
            t = col[...].T
            st_send[i, 0:8, :] = t[0:8, :]
            st_send[i, 8:16, :] = t[64:72, :]

        def normalize(i):
            a = st_send[i]
            b = st_recv[i]
            ma, va = a[0:8, :], a[8:16, :]
            mb, vb = b[0:8, :], b[8:16, :]
            mean = 0.5 * (ma + mb)
            dl = ma - mb
            m2 = va + vb + dl * dl * (N / 2.0)
            rstd = 1.0 / jnp.sqrt(m2 * (1.0 / n_total) + EPS)
            mu[...] = jnp.broadcast_to(mean[0:1, :], (128, R)).T
            rs[...] = jnp.broadcast_to(rstd[0:1, :], (128, R)).T

            def chunk(c, _):
                r0 = pl.multiple_of(c * NCH, NCH)
                m = mu[pl.ds(r0, NCH), :]
                r = rs[pl.ds(r0, NCH), :]
                for t in range(N // 128):
                    cs = pl.ds(t * 128, 128)
                    xs = xbuf[i, pl.ds(r0, NCH), cs]
                    gg = jnp.tile(gb[0:8, cs], (NCH // 8, 1))
                    bb = jnp.tile(gb[8:16, cs], (NCH // 8, 1))
                    y = (xs - m) * r * gg + bb
                    o_ref[pl.ds(pl.multiple_of(i * R + r0, NCH), NCH), cs] = y.astype(out_dtype)
                return 0
            lax.fori_loop(0, R // NCH, chunk, 0)

        rd(0).wait()
        rd(D).start()
        stats(0)
        pl.semaphore_wait(bar, 1)
        xch(0).start()
        cg.wait()
        cb.wait()
        g1 = gb1[0, :].reshape(N // 128, 128)
        b1 = gb1[1, :].reshape(N // 128, 128)
        for t in range(N // 128):
            gb[0:8, t * 128:(t + 1) * 128] = jnp.broadcast_to(g1[t:t + 1, :], (8, 128))
            gb[8:16, t * 128:(t + 1) * 128] = jnp.broadcast_to(b1[t:t + 1, :], (8, 128))

        def step(i, _):
            rd(i).wait()

            @pl.when(i + D < NB)
            def _():
                rd(i + D).start()
            stats(i)
            xch(i).start()
            xch(i - LAG).wait_recv()
            normalize(i - LAG)
            return 0

        lax.fori_loop(1, NB, step, 0)
        for j in range(NB - LAG, NB):
            xch(j).wait_recv()
            normalize(j)
        for i in range(NB):
            xch(i).wait_send()

    return pl.pallas_call(
        body,
        out_shape=pltpu.VMEM((M, N), out_dtype),
        in_specs=[pl.BlockSpec(memory_space=pl.ANY)] * 3,
        out_specs=pl.BlockSpec(memory_space=pltpu.VMEM),
        scratch_shapes=[
            pltpu.VMEM((NB, R, N), jnp.float32),
            pltpu.VMEM((2, N), jnp.float32),
            pltpu.VMEM((16, N), jnp.float32),
            pltpu.VMEM((R, 128), jnp.float32),
            pltpu.VMEM((R, 128), jnp.float32),
            pltpu.VMEM((R, 128), jnp.float32),
            pltpu.VMEM((NB, 16, R), jnp.float32),
            pltpu.VMEM((NB, 16, R), jnp.float32),
            pltpu.SemaphoreType.DMA((NB,)),
            pltpu.SemaphoreType.DMA((2,)),
            pltpu.SemaphoreType.DMA((NB,)),
            pltpu.SemaphoreType.DMA((NB,)),
        ],
        compiler_params=pltpu.CompilerParams(vmem_limit_bytes=60 * 2**20, collective_id=0),
    )(x, gamma, beta)
```

```python
import functools

import jax
import jax.numpy as jnp
from jax import lax
from jax.experimental import pallas as pl
from jax.experimental.pallas import tpu as pltpu

EPS = 1e-5
LANES = 128
SUB = 8

BLOCK = 512
TAIL = (256, 128, 96, 32)
DEPTH = 4
CHUNK = 256
HOLD = 4


def pallas_dist_layernorm_xy_m6144_n2048_kernel(
    x: jax.Array,
    gamma: jax.Array,
    beta: jax.Array,
):
    m, n = x.shape
    n_bulk = (m - sum(TAIL)) // BLOCK
    sizes = [BLOCK] * n_bulk + list(TAIL)
    assert sum(sizes) == m and n % LANES == 0 and n_bulk > DEPTH
    assert all(s % SUB == 0 and s <= SUB * LANES and s % min(s, CHUNK) == 0 for s in sizes)
    starts = [sum(sizes[:i]) for i in range(len(sizes))]
    n_blocks = len(sizes)
    n_local = float(n)
    n_total = 2.0 * n

    def body(x_hbm, g_hbm, b_hbm, o_ref, xbuf, gb_raw, gb, st_send, st_recv):
        pl.run_scoped(
            functools.partial(run, x_hbm, g_hbm, b_hbm, o_ref, xbuf, gb_raw, gb, st_send, st_recv),
            rd_sem=pltpu.SemaphoreType.DMA((DEPTH,)),
            gb_sem=pltpu.SemaphoreType.DMA,
            send_sem=pltpu.SemaphoreType.DMA,
            recv_sem=pltpu.SemaphoreType.DMA((n_blocks,)),
        )

    def run(x_hbm, g_hbm, b_hbm, o_ref, xbuf, gb_raw, gb, st_send, st_recv,
            rd_sem, gb_sem, send_sem, recv_sem):
        peer = (lax.axis_index("x"), 1 - lax.axis_index("y"))
        lane = lax.broadcasted_iota(jnp.int32, (SUB, LANES), 1)

        def read(i, size=None):
            if size is None:
                size, r0, slot = sizes[i], starts[i], i % DEPTH
            else:
                r0, slot = pl.multiple_of(i * BLOCK, SUB), lax.rem(i, DEPTH)
            return pltpu.make_async_copy(
                x_hbm.at[pl.ds(r0, size), :], xbuf.at[pl.ds(r0, size), :], rd_sem.at[slot])

        def exchange(i):
            return pltpu.make_async_remote_copy(
                src_ref=st_send.at[i], dst_ref=st_recv.at[i],
                send_sem=send_sem, recv_sem=recv_sem.at[i],
                device_id=peer, device_id_type=pl.DeviceIdType.MESH)

        def stats(i, row0, size):
            ch = min(CHUNK, size)

            def chunk(c, carry):
                mm, mv = carry
                xs = xbuf[pl.ds(pl.multiple_of(row0 + c * ch, SUB), ch), :]
                mean = jnp.sum(xs, axis=-1, keepdims=True) * (1.0 / n_local)
                d = xs - mean
                m2 = jnp.sum(d * d, axis=-1, keepdims=True)
                mean = jnp.broadcast_to(mean, (ch, LANES))
                m2 = jnp.broadcast_to(m2, (ch, LANES))
                for k in range(ch // SUB):
                    sel = lane == c * (ch // SUB) + k
                    mm = jnp.where(sel, mean[SUB * k:SUB * (k + 1)], mm)
                    mv = jnp.where(sel, m2[SUB * k:SUB * (k + 1)], mv)
                return mm, mv

            zero = jnp.zeros((SUB, LANES), jnp.float32)
            if size == ch:
                mm, mv = chunk(0, (zero, zero))
            else:
                mm, mv = lax.fori_loop(0, size // ch, chunk, (zero, zero))
            st_send[i, 0:SUB, :] = mm
            st_send[i, SUB:2 * SUB, :] = mv

        def normalize(i, row0, size):
            ch = min(CHUNK, size)
            mine, other = st_send[i], st_recv[i]
            mean = 0.5 * (mine[0:SUB] + other[0:SUB])
            delta = mine[0:SUB] - other[0:SUB]
            m2 = mine[SUB:] + other[SUB:] + delta * delta * (n_local * n_local / n_total)
            rstd = 1.0 / jnp.sqrt(m2 * (1.0 / n_total) + EPS)

            def chunk(c, carry):
                r0 = pl.multiple_of(row0 + c * ch, SUB)
                mu, rs = [], []
                for k in range(ch // SUB):
                    sel = lane == c * (ch // SUB) + k
                    mu.append(jnp.sum(jnp.where(sel, mean, 0.0), axis=-1, keepdims=True))
                    rs.append(jnp.sum(jnp.where(sel, rstd, 0.0), axis=-1, keepdims=True))
                for t in range(n // LANES):
                    cols = pl.ds(t * LANES, LANES)
                    g, b = gb[0:SUB, cols], gb[SUB:, cols]
                    for k in range(ch // SUB):
                        rows = pl.ds(pl.multiple_of(r0 + SUB * k, SUB), SUB)
                        o_ref[rows, cols] = (xbuf[rows, cols] - mu[k]) * rs[k] * g + b
                return carry

            if size == ch:
                chunk(0, 0)
            else:
                lax.fori_loop(0, size // ch, chunk, 0)

        read(0).start()
        pltpu.make_async_copy(g_hbm, gb_raw.at[0], gb_sem).start()
        pltpu.make_async_copy(b_hbm, gb_raw.at[1], gb_sem).start()
        for i in range(1, DEPTH):
            read(i).start()
        barrier = pltpu.get_barrier_semaphore()
        pl.semaphore_signal(barrier, inc=1, device_id=peer, device_id_type=pl.DeviceIdType.MESH)

        read(0).wait()
        read(DEPTH).start()
        stats(0, 0, BLOCK)
        pl.semaphore_wait(barrier, 1)
        exchange(0).start()
        pltpu.make_async_copy(gb_raw, gb_raw, gb_sem).wait()
        g_rows = gb_raw[0, :].reshape(n // LANES, LANES)
        b_rows = gb_raw[1, :].reshape(n // LANES, LANES)
        for t in range(n // LANES):
            cols = pl.ds(t * LANES, LANES)
            gb[0:SUB, cols] = jnp.broadcast_to(g_rows[t:t + 1], (SUB, LANES))
            gb[SUB:, cols] = jnp.broadcast_to(b_rows[t:t + 1], (SUB, LANES))

        def bulk_step(i, carry):
            read(i, BLOCK).wait()

            @pl.when(i + DEPTH < n_bulk)
            def _():
                read(i + DEPTH, BLOCK).start()

            for j in range(n_bulk - DEPTH, n_bulk):
                if j + DEPTH < n_blocks:
                    @pl.when(i == j)
                    def _():
                        read(j + DEPTH).start()

            stats(i, i * BLOCK, BLOCK)
            exchange(i).start()
            exchange(i - 1).wait_recv()
            normalize(i - 1, (i - 1) * BLOCK, BLOCK)
            return carry

        lax.fori_loop(1, n_bulk, bulk_step, 0)

        done = n_bulk - 1
        for i in range(n_bulk, n_blocks):
            read(i).wait()
            if i + DEPTH < n_blocks:
                read(i + DEPTH).start()
            stats(i, starts[i], sizes[i])
            exchange(i).start()
            if i - 1 < n_blocks - HOLD:
                exchange(i - 1).wait_recv()
                normalize(i - 1, starts[i - 1], sizes[i - 1])
                done = i
        for i in range(done, n_blocks):
            exchange(i).wait_recv()
            normalize(i, starts[i], sizes[i])
        pltpu.make_async_copy(st_send, st_send, send_sem).wait()

    return pl.pallas_call(
        body,
        out_shape=pltpu.VMEM((m, n), jnp.float32),
        in_specs=[pl.BlockSpec(memory_space=pl.ANY)] * 3,
        out_specs=pl.BlockSpec(memory_space=pltpu.VMEM),
        scratch_shapes=[
            pltpu.VMEM((m, n), jnp.float32),
            pltpu.VMEM((2, n), jnp.float32),
            pltpu.VMEM((2 * SUB, n), jnp.float32),
            pltpu.VMEM((n_blocks, 2 * SUB, LANES), jnp.float32),
            pltpu.VMEM((n_blocks, 2 * SUB, LANES), jnp.float32),
        ],
        compiler_params=pltpu.CompilerParams(
            vmem_limit_bytes=60 * 2**20, collective_id=0),
    )(x, gamma, beta)
```
